```python
import numpy as np

kernel_name = "dist_moe_cap_ep_outshard_n2048_d512_e8_h1024"

def setup_inputs():
    x = np.random.randn(2048, 512).astype(np.float32)
    router_W = np.random.randn(512, 32).astype(np.float32) * 0.1
    scores64 = x.astype(np.float64) @ router_W.astype(np.float64)
    route_idx = np.argsort(-scores64, axis=-1)[:, :1].astype(np.int32)
    expert_W = np.random.randn(32, 512, 1024).astype(np.float32) * 0.02
    return {"x": x, "router_W": router_W, "route_idx": route_idx, "expert_W": expert_W}

def reference(x, router_W, route_idx, expert_W):
    counts = np.zeros(32, dtype=np.int64)
    out = np.zeros((2048, 1024), dtype=np.float32)
    for i in range(2048):
        e = int(route_idx[i, 0])
        if counts[e] < 51:
            out[i] = x[i] @ expert_W[e]
            counts[e] += 1
    return out
```

```python
import jax
import jax.numpy as jnp
from jax import lax
from jax.experimental import pallas as pl
from jax.experimental.pallas import tpu as pltpu

N_TOK, D, H = 2048, 512, 1024
N_DEV, E_LOC, N_EXP, CAP = 4, 8, 32, 51
ROWS = N_TOK // N_DEV
NBLK = N_TOK // 128
SLOTS = 64
LSLOTS = 56

SEG = 4
CAPB = 416
DSTEP = 32
assert CAPB % DSTEP == 0 and CAPB >= E_LOC * (-(-CAP // SEG) * SEG)
SEND0 = N_DEV * CAPB
ZERO = 2 * N_DEV * CAPB
TRASH = ZERO + 1
NBUF = ZERO + 8

T_QD, T_QC, T_GD, T_GC, T_CUM, T_QA, T_GL = 0, 4, 8, 16, 24, 56, 60
T_ROWS = 64

LCAP = 56
LTRASH = 2 * N_DEV * LCAP
LROWS = LTRASH + 8

NTD = D // 2 // 128
NTC = H // 2 // 128

LAST_SPLIT = tuple((256 * j, 256 * j + 256) for j in range(NTC))

_F32, _BF16, _I32 = jnp.float32, jnp.bfloat16, jnp.int32

_DEBUG_CHECKS_OFF = {k: True for k in ("disable_semaphore_checks",)
                     if hasattr(pltpu.CompilerParams, k)}


def _pack_pairs(v):
    k = v.shape[1] // 2
    vr = v.astype(_BF16).astype(_F32)
    lo = lax.shift_right_logical(lax.bitcast_convert_type(vr[:, :k], _I32), 16)
    hi = lax.bitcast_convert_type(vr[:, k:], _I32)
    return hi | lo


def _unpack_lo(p):
    return lax.bitcast_convert_type(lax.shift_left(p, 16), _F32)


def _unpack_hi(p):
    return lax.bitcast_convert_type(p & jnp.int32(-65536), _F32)


def _sel4(me, xs):
    return jnp.where(me == 0, xs[0], jnp.where(me == 1, xs[1], jnp.where(me == 2, xs[2], xs[3])))


def _routing_table(r, me):
    e_i = lax.broadcasted_iota(_I32, (N_EXP, 128), 0)
    lane = lax.broadcasted_iota(_I32, (N_EXP, 128), 1)
    lane_f = lane.astype(_F32)
    grp = lax.shift_right_logical(e_i, 3)

    ots = [r[b:b + 1, :] == e_i for b in range(NBLK)]
    ot_all = jnp.concatenate([jnp.where(o, 1.0, 0.0) for o in ots], axis=0).astype(_BF16)
    ui = lax.broadcasted_iota(_I32, (128, 256), 0)
    uj = lax.broadcasted_iota(_I32, (128, 256), 1)
    u = jnp.where((uj >= 128) | (ui < uj), 1.0, 0.0).astype(_BF16)
    m = jnp.dot(ot_all, u, preferred_element_type=_F32)

    off = jnp.zeros((N_EXP, 128), _F32)
    ranks, bounds = [], []
    for b in range(NBLK):
        if b % 4 == 0:
            bounds.append(jnp.minimum(off, float(CAP)))
        c = m[32 * b:32 * b + 32, :128] + off
        ranks.append(jnp.sum(jnp.where(ots[b], c, 0.0), axis=0, keepdims=True))
        off = off + m[32 * b:32 * b + 32, 128:]
    bounds.append(jnp.minimum(off, float(CAP)))

    gi = lax.broadcasted_iota(_I32, (N_EXP, N_EXP), 0)
    gj = lax.broadcasted_iota(_I32, (N_EXP, N_EXP), 1)
    g = jnp.where((gj < gi) & ((gj >> 3) == (gi >> 3)), 1.0, 0.0).astype(_BF16)

    ns = [bounds[t + 1] - bounds[t] for t in range(N_DEV)]
    nps = [jnp.floor((n + float(SEG - 1)) * (1.0 / SEG)) * float(SEG) for n in ns]
    bases = [jnp.dot(g, n.astype(_BF16), preferred_element_type=_F32) for n in nps]

    qds, qcs, qas = [], [], []
    grp_f = grp.astype(_F32) * float(CAPB)
    for b in range(NBLK):
        t = b // 4
        val = bases[t] - bounds[t] + grp_f
        pos = jnp.sum(jnp.where(ots[b], val, 0.0), axis=0, keepdims=True) + ranks[b]
        kept = ranks[b] < float(CAP)
        remote = lax.shift_right_logical(r[b:b + 1, :], 3) != t
        qcs.append(jnp.where(kept, pos, float(ZERO)))
        late = remote & ((r[b:b + 1, :] & (E_LOC - 1)) >= E_LOC - 2)
        qas.append(jnp.where(kept & jnp.logical_not(late), pos, float(ZERO)))
        qds.append(jnp.where(kept, pos + jnp.where(remote, float(SEND0), 0.0), float(TRASH)))
    qd = _sel4(me, [jnp.concatenate(qds[4 * t:4 * t + 4], axis=0) for t in range(N_DEV)])
    qc = _sel4(me, [jnp.concatenate(qcs[4 * t:4 * t + 4], axis=0) for t in range(N_DEV)])
    qa = _sel4(me, [jnp.concatenate(qas[4 * t:4 * t + 4], axis=0) for t in range(N_DEV)])

    gd = jnp.full((N_EXP, 128), float(ZERO), _F32)
    gc = jnp.full((N_EXP, 128), float(TRASH), _F32)
    gl = jnp.full((N_EXP, 128), float(LTRASH), _F32)
    cum = jnp.zeros((N_EXP, 128), _F32)
    for t in range(N_DEV):
        msk = (lane_f >= bounds[t]) & (lane_f < bounds[t + 1])
        gl = jnp.where(msk & (grp != t), lane_f - bounds[t] + float((N_DEV + t) * LCAP), gl)
        pos = bases[t] + lane_f - bounds[t] + float(t * CAPB)
        gd = jnp.where(msk, pos, gd)
        gc = jnp.where(msk, pos + jnp.where(grp == t, 0.0, float(SEND0)), gc)
        cum = jnp.where(lane == t, bases[t], cum)
        cum = jnp.where(lane == N_DEV + t, nps[t], cum)
        cum = jnp.where(lane == 2 * N_DEV + t, ns[t], cum)
    gc = jnp.where(((e_i & (E_LOC - 1)) == E_LOC - 1) & (gl != float(LTRASH)), float(TRASH), gc)
    gd = _sel4(me, [gd[8 * s:8 * s + 8] for s in range(N_DEV)])
    gc = _sel4(me, [gc[8 * s:8 * s + 8] for s in range(N_DEV)])
    gl = _sel4(me, [gl[8 * s + 7:8 * s + 8] for s in range(N_DEV)])

    tab = jnp.concatenate([qd * float(NTD), qc, gd * float(NTD), gc * float(NTC), cum,
                           qa * float(NTC), gl, gl, gl, gl], axis=0)
    return tab.astype(_I32)


def _tile_row(i, nt):
    return pl.ds((i // 8) * nt * 8 + i % 8, nt, stride=8)


def _store_tiles(ref, val, nt):
    for g in range(val.shape[0] // 8):
        for j in range(nt):
            ref[pl.ds((g * nt + j) * 8, 8), :] = val[8 * g:8 * g + 8, 128 * j:128 * j + 128]


def _body(x_hbm, r_hbm, w_hbm, out_ref,
          w_v, xq_v, xp_v, r_v, tab_v, tab_s, inv_s, dbuf, cbuf, lbuf, xg, yb,
          w_sems, x_sem, r_sem, tab_sem,
          dsend_sems, csend_sems, lsend_sems, drecv_sems, crecv_sems, lrecv_sems):
    me = lax.axis_index("i")

    r_cp = pltpu.make_async_copy(r_hbm, r_v, r_sem)
    r_cp.start()
    x_cp = pltpu.make_async_copy(x_hbm.at[pl.ds(me * ROWS, ROWS)], xq_v, x_sem)
    x_cp.start()
    w_cps = [[((0, H), pltpu.make_async_copy(w_hbm.at[p], w_v.at[p], w_sems.at[p]))]
             for p in range(E_LOC - 1)]
    w_cps.append([((c0, c1), pltpu.make_async_copy(
        w_hbm.at[E_LOC - 1, :, pl.ds(c0, c1 - c0)], w_v.at[E_LOC - 1, :, pl.ds(c0, c1 - c0)],
        w_sems.at[E_LOC - 1 + k])) for k, (c0, c1) in enumerate(LAST_SPLIT)])

    barrier = pltpu.get_barrier_semaphore()
    for k in range(1, N_DEV):
        pl.semaphore_signal(barrier, inc=1, device_id=((me + k) % N_DEV,),
                            device_id_type=pl.DeviceIdType.MESH)

    dbuf[pl.ds(ZERO * NTD, 8 * NTD), :] = jnp.zeros((8 * NTD, 128), _I32)
    cbuf[pl.ds(ZERO * NTC, 8 * NTC), :] = jnp.zeros((8 * NTC, 128), _I32)
    xg[...] = jnp.zeros_like(xg)

    r_cp.wait()
    for cps in w_cps:
        for _, cp in cps:
            cp.start()
    tab_v[...] = _routing_table(r_v[...], me)
    tab_cp = pltpu.make_async_copy(tab_v, tab_s, tab_sem)
    tab_cp.start()

    x_cp.wait()
    tab_cp.wait()

    _store_tiles(xp_v, _pack_pairs(xq_v[...]), NTD)

    def l1():
        for i in range(ROWS):
            idx = tab_s[T_QD + i // 128, i % 128]
            dbuf[pl.ds(idx, NTD), :] = xp_v[_tile_row(i, NTD), :]
            inv_s[tab_s[T_QC + i // 128, i % 128]] = (i // 8) * 64 + i % 8
    l1()

    pl.semaphore_wait(barrier, N_DEV - 1)

    def rows_of(buf, nt, region, start, size):
        return buf.at[pl.ds(pl.multiple_of((region * CAPB + start) * nt, 8), size * nt)]

    def d_copy(peer, size, src_region, dst_region, sem_idx):
        return pltpu.make_async_remote_copy(
            src_ref=rows_of(dbuf, NTD, src_region, 0, size), dst_ref=rows_of(dbuf, NTD, dst_region, 0, size),
            send_sem=dsend_sems.at[sem_idx], recv_sem=drecv_sems.at[sem_idx],
            device_id=(peer,), device_id_type=pl.DeviceIdType.MESH)

    def c_copy(peer, start, size, src_region, dst_region, sem_idx):
        return pltpu.make_async_remote_copy(
            src_ref=rows_of(cbuf, NTC, src_region, start, size),
            dst_ref=rows_of(cbuf, NTC, dst_region, start, size),
            send_sem=csend_sems.at[sem_idx], recv_sem=crecv_sems.at[sem_idx],
            device_id=(peer,), device_id_type=pl.DeviceIdType.MESH)

    def l_copy(j, peer, size, src_region, dst_region, sl):
        def rows(region):
            return lbuf.at[pl.ds(pl.multiple_of(j * LROWS + region * LCAP, 8), size)]
        return pltpu.make_async_remote_copy(
            src_ref=rows(src_region), dst_ref=rows(dst_region),
            send_sem=lsend_sems.at[sl * NTC + j], recv_sem=lrecv_sems.at[sl * NTC + j],
            device_id=(peer,), device_id_type=pl.DeviceIdType.MESH)

    def for_lsize(n, fn):
        steps = lax.shift_right_logical(n + 7, 3)
        for q in range(1, LCAP // 8 + 1):
            pl.when(steps == q)(lambda q=q: fn(q * 8))

    def for_dsize(n, fn):
        steps = lax.shift_right_logical(n + (DSTEP - 1), 5)
        for q in range(1, CAPB // DSTEP + 1):
            pl.when(steps == q)(lambda q=q: fn(q * DSTEP))

    def for_csize(n, fn):
        for q in range(SEG, CAP + SEG, SEG):
            pl.when(n == q)(lambda q=q: fn(q))

    ks = (2, 1, 3)
    peers = [(me + k) % N_DEV for k in ks]
    out_slot = [N_DEV - k - 1 for k in ks]
    in_slot = [k - 1 for k in ks]
    n_tok_pair = [tab_s[T_CUM + 8 * s + 7, me] + tab_s[T_CUM + 8 * s + 7, N_DEV + me] for s in peers]
    n_exp_pair = [tab_s[T_CUM + 8 * me + 7, t] + tab_s[T_CUM + 8 * me + 7, N_DEV + t] for t in peers]

    for s, n, sl in zip(peers, n_tok_pair, out_slot):
        for_dsize(n, lambda size, s=s, sl=sl: d_copy(s, size, N_DEV + s, me, sl).start())

    for t, n, sl in zip(peers, n_exp_pair, in_slot):
        for_dsize(n, lambda size, t=t, sl=sl: d_copy(t, size, t, t, sl).wait_recv())

    def cwait(p, c):
        for s, sl in zip(peers, in_slot):
            st = tab_s[T_CUM + 8 * s + p, me]
            for_csize(tab_s[T_CUM + 8 * s + p, N_DEV + me],
                      lambda sz, s=s, sl=sl, st=st: c_copy(s, st, sz, s, s, sl * (E_LOC - 1) + p).wait_recv())
        return c

    def csw(p, c):
        for t, sl in zip(peers, out_slot):
            st = tab_s[T_CUM + 8 * me + p, t]
            for_csize(tab_s[T_CUM + 8 * me + p, N_DEV + t],
                      lambda sz, t=t, sl=sl, st=st: c_copy(t, st, sz, N_DEV + t, me, sl * (E_LOC - 1) + p).wait_send())
        return c

    for p in range(E_LOC):
        def l2(p=p):
            for j in range(LSLOTS):
                idx = tab_s[T_GD + p, j]
                xg[_tile_row(j, NTD), :] = dbuf[pl.ds(idx, NTD), :]
        l2()

        if p == E_LOC - 4:
            for s, n, sl in zip(peers, n_tok_pair, out_slot):
                for_dsize(n, lambda size, s=s, sl=sl: d_copy(s, size, N_DEV + s, me, sl).wait_send())
        if p >= E_LOC - 3:
            lax.fori_loop(2 * (p - E_LOC + 3), 2 * (p - E_LOC + 4), csw, 0)
            lax.fori_loop(2 * (p - E_LOC + 3), min(2 * (p - E_LOC + 4), 5), cwait, 0)

        xpk = jnp.concatenate(
            [jnp.concatenate([xg[pl.ds((g * NTD + j) * 8, 8), :] for g in range(SLOTS // 8)], axis=0)
             for j in range(NTD)], axis=1)
        xb = jnp.concatenate([_unpack_lo(xpk), _unpack_hi(xpk)], axis=1).astype(_BF16)

        last = p == E_LOC - 1
        n_last = [tab_s[T_CUM + 8 * me + E_LOC - 1, 2 * N_DEV + t] for t in peers]

        for (c0, c1), cp in w_cps[p]:
            cp.wait()

            def mm(p=p, c0=c0, c1=c1):
                y = jnp.dot(xb, w_v[p, :, c0:c1].astype(_BF16), preferred_element_type=_F32)
                for j in range(c0 // 256, c1 // 256):
                    pk = _pack_pairs(y[:, 256 * j - c0:256 * j - c0 + 256])
                    for g in range(SLOTS // 8):
                        yb[pl.ds((g * NTC + j) * 8, 8), :] = pk[8 * g:8 * g + 8, :]
            mm()

            if last:
                jt = c0 // 256
                for j in range(LSLOTS):
                    idx = tab_s[T_GL, j]
                    lbuf[pl.ds(jt * LROWS + idx, 1), :] = yb[pl.ds((j // 8) * NTC * 8 + jt * 8 + j % 8, 1), :]
                for t, sl, n in zip(peers, out_slot, n_last):
                    for_lsize(n, lambda sz, t=t, sl=sl, jt=jt: l_copy(jt, t, sz, N_DEV + t, me, sl).start())

        def l3(p=p):
            for j in range(LSLOTS):
                idx = tab_s[T_GC + p, j]
                cbuf[pl.ds(idx, NTC), :] = yb[_tile_row(j, NTC), :]
        l3()

        if not last:
            for t, sl in zip(peers, out_slot):
                st = tab_s[T_CUM + 8 * me + p, t]
                for_csize(tab_s[T_CUM + 8 * me + p, N_DEV + t], lambda sz, t=t, sl=sl, st=st, p=p: c_copy(t, st, sz, N_DEV + t, me, sl * (E_LOC - 1) + p).start())

    def put_row(orow, v):
        out_ref[pl.ds(orow, NTC, stride=16), :] = _unpack_lo(v)
        out_ref[pl.ds(orow + 8, NTC, stride=16), :] = _unpack_hi(v)

    lax.fori_loop(E_LOC - 3, E_LOC - 2, cwait, 0)

    def l4():
        for i in range(ROWS):
            idx = tab_s[T_QA + i // 128, i % 128]
            put_row((i // 8) * 64 + i % 8, cbuf[pl.ds(idx, NTC), :])
    l4()

    lax.fori_loop(E_LOC - 2, E_LOC - 1, csw, 0)

    def patch_all(p, put):
        for s in peers:
            st = s * CAPB + tab_s[T_CUM + 8 * s + p, me]
            n = tab_s[T_CUM + 8 * s + p, 2 * N_DEV + me]

            def patch(k, c, s=s, st=st, n=n):
                for jj in range(SEG):
                    j = jnp.minimum(k * SEG + jj, n - 1)
                    put(inv_s[st + j], s * LCAP + j, st + j)
                return c
            lax.fori_loop(0, lax.shift_right_logical(n + (SEG - 1), 2), patch, 0)

    lax.fori_loop(E_LOC - 2, E_LOC - 1, cwait, 0)
    patch_all(E_LOC - 2, lambda orow, lrow, row: put_row(orow, cbuf[pl.ds(row * NTC, NTC), :]))

    n_in = [tab_s[T_CUM + 8 * s + E_LOC - 1, 2 * N_DEV + me] for s in peers]

    def put_tiles(jts):
        def put(orow, lrow, row):
            for jt in jts:
                v = lbuf[pl.ds(jt * LROWS + lrow, 1), :]
                out_ref[pl.ds(orow + 16 * jt, 1), :] = _unpack_lo(v)
                out_ref[pl.ds(orow + 16 * jt + 8, 1), :] = _unpack_hi(v)
        return put

    def lwait(jts):
        for jt in jts:
            for s, sl, n in zip(peers, in_slot, n_in):
                for_lsize(n, lambda sz, s=s, sl=sl, jt=jt: l_copy(jt, s, sz, s, s, sl).wait_recv())

    lwait(range(NTC - 1))
    patch_all(E_LOC - 1, put_tiles(range(NTC - 1)))
    for jt in range(NTC):
        for t, sl, n in zip(peers, out_slot, n_last):
            for_lsize(n, lambda sz, t=t, sl=sl, jt=jt: l_copy(jt, t, sz, N_DEV + t, me, sl).wait_send())
    lwait([NTC - 1])
    patch_all(E_LOC - 1, put_tiles([NTC - 1]))


def pallas_dist_moe_cap_ep_outshard_n2048_d512_e8_h1024_kernel(
    x: jax.Array,
    router_W: jax.Array,
    route_idx: jax.Array,
    expert_W: jax.Array,
):
    del router_W
    r = route_idx.astype(_I32).reshape(NBLK, 128)
    any_spec = pl.BlockSpec(memory_space=pl.ANY)
    out = pl.pallas_call(
        _body,
        out_shape=jax.ShapeDtypeStruct((ROWS * H // 128, 128), _F32),
        in_specs=[any_spec, any_spec, any_spec],
        out_specs=pl.BlockSpec(memory_space=pltpu.VMEM),
        scratch_shapes=[
            pltpu.VMEM((E_LOC, D, H), _F32),
            pltpu.VMEM((ROWS, D), _F32),
            pltpu.VMEM((ROWS * NTD, 128), _I32),
            pltpu.VMEM((NBLK, 128), _I32),
            pltpu.VMEM((T_ROWS, 128), _I32),
            pltpu.SMEM((T_ROWS, 128), _I32),
            pltpu.SMEM((NBUF,), _I32),
            pltpu.VMEM((NBUF * NTD, 128), _I32),
            pltpu.VMEM((NBUF * NTC, 128), _I32),
            pltpu.VMEM((NTC * LROWS, 128), _I32),
            pltpu.VMEM((SLOTS * NTD, 128), _I32),
            pltpu.VMEM((SLOTS * NTC, 128), _I32),
            pltpu.SemaphoreType.DMA((E_LOC - 1 + len(LAST_SPLIT),)),
            pltpu.SemaphoreType.DMA,
            pltpu.SemaphoreType.DMA,
            pltpu.SemaphoreType.DMA,
            pltpu.SemaphoreType.DMA((N_DEV - 1,)),
            pltpu.SemaphoreType.DMA(((N_DEV - 1) * (E_LOC - 1),)),
            pltpu.SemaphoreType.DMA(((N_DEV - 1) * NTC,)),
            pltpu.SemaphoreType.DMA((N_DEV - 1,)),
            pltpu.SemaphoreType.DMA(((N_DEV - 1) * (E_LOC - 1),)),
            pltpu.SemaphoreType.DMA(((N_DEV - 1) * NTC,)),
        ],
        compiler_params=pltpu.CompilerParams(
            collective_id=0, vmem_limit_bytes=64 * 1024 * 1024, **_DEBUG_CHECKS_OFF),
    )(x, r, expert_W)
    return out.reshape(ROWS // 8, H // 128, 8, 128).transpose(0, 2, 1, 3).reshape(ROWS, H)
```
